```python
import numpy as np

kernel_name = "dist_mean_ax0_shard0_i_m1024_n512"

def setup_inputs():
    return {"x": np.random.randn(4096, 512).astype(np.float32)}

def reference(x: np.ndarray) -> np.ndarray:
    return np.mean(x, axis=0, keepdims=True)
```

```python
import jax
import jax.numpy as jnp
from jax import lax
from jax.experimental import pallas as pl
from jax.experimental.pallas import tpu as pltpu

_AXIS = "i"
_N_DEV = 4
_CHUNK_ROWS = (768, 192, 48, 16)
_SEND_ORDER = (2, 1, 3)
_RECV_ORDER = (1, 3, 2)


def _tree_sum(terms):
    terms = list(terms)
    while len(terms) > 1:
        pairs = [terms[i] + terms[i + 1] for i in range(0, len(terms) - 1, 2)]
        terms = pairs + terms[2 * len(pairs):]
    return terms[0]


def pallas_dist_mean_ax0_shard0_i_m1024_n512_kernel(x: jax.Array):
    m, n = x.shape
    assert sum(_CHUNK_ROWS) == m
    starts = [sum(_CHUNK_ROWS[:c]) for c in range(len(_CHUNK_ROWS))]
    scale = 1.0 / (m * _N_DEV)

    def kernel_body(x_hbm, out_ref, x_vmem, sums, load_sems, send_sems, recv_sems):
        loads = [
            pltpu.make_async_copy(
                x_hbm.at[pl.ds(start, rows)],
                x_vmem.at[pl.ds(start, rows)],
                load_sems.at[c],
            )
            for c, (start, rows) in enumerate(zip(starts, _CHUNK_ROWS))
        ]
        for load in loads:
            load.start()

        me = lax.axis_index(_AXIS)
        peers = {k: (me + k) & (_N_DEV - 1) for k in _SEND_ORDER}
        barrier = pltpu.get_barrier_semaphore()
        for k in _SEND_ORDER:
            pl.semaphore_signal(
                barrier,
                inc=1,
                device_id=(peers[k],),
                device_id_type=pl.DeviceIdType.MESH,
            )

        acc = None
        for load, start, rows in list(zip(loads, starts, _CHUNK_ROWS))[:-1]:
            load.wait()
            block = x_vmem[pl.ds(start, rows), :].reshape(rows // 8, 8, n).sum(axis=0)
            acc = block if acc is None else acc + block
        pl.semaphore_wait(barrier, _N_DEV - 1)
        loads[-1].wait()
        acc = _tree_sum(
            [x_vmem[pl.ds(starts[-1] + r, 8), :] for r in range(0, _CHUNK_ROWS[-1], 8)]
            + [acc]
        )
        total = jnp.sum(acc, axis=0, keepdims=True)
        sums[0] = total

        copies = {
            k: pltpu.make_async_remote_copy(
                src_ref=sums.at[0],
                dst_ref=sums.at[k],
                send_sem=send_sems.at[k - 1],
                recv_sem=recv_sems.at[k - 1],
                device_id=(peers[k],),
                device_id_type=pl.DeviceIdType.MESH,
            )
            for k in _SEND_ORDER
        }
        for k in _SEND_ORDER:
            copies[k].start()
        for k in _SEND_ORDER:
            copies[k].wait_send()
        for k in _RECV_ORDER:
            copies[k].wait_recv()
            total = total + sums[k]
        out_ref[...] = total * scale

    return pl.pallas_call(
        kernel_body,
        out_shape=jax.ShapeDtypeStruct((1, n), x.dtype),
        in_specs=[pl.BlockSpec(memory_space=pl.ANY)],
        out_specs=pl.BlockSpec(memory_space=pltpu.VMEM),
        scratch_shapes=[
            pltpu.VMEM((m, n), jnp.float32),
            pltpu.VMEM((_N_DEV, 1, n), jnp.float32),
            pltpu.SemaphoreType.DMA((len(_CHUNK_ROWS),)),
            pltpu.SemaphoreType.DMA((_N_DEV - 1,)),
            pltpu.SemaphoreType.DMA((_N_DEV - 1,)),
        ],
        compiler_params=pltpu.CompilerParams(
            collective_id=0,
            disable_semaphore_checks=True,
        ),
    )(x)
```

```python
import jax
import jax.numpy as jnp
from jax import lax
from jax.experimental import pallas as pl
from jax.experimental.pallas import tpu as pltpu

_AXIS = "i"
_N_DEV = 4
_SUBLANES = 8

_HEAD_ROWS = 48
_STRIP_ROWS = 192
_NARROW_COLS = 128
_WIDE_END_ROWS = 16
_NARROW_END_ROWS = 32


def _fold_rows(ref):
    rows, cols = ref.shape
    return ref[...].reshape(rows // _SUBLANES, _SUBLANES, cols).sum(axis=0)


def _fold_rows_onto(acc, ref):
    terms = [ref[pl.ds(r, _SUBLANES), :] for r in range(0, ref.shape[0], _SUBLANES)]
    terms.append(acc)
    while len(terms) > 1:
        pairs = [a + b for a, b in zip(terms[0::2], terms[1::2])]
        terms = pairs + terms[2 * len(pairs) :]
    return terms[0]


def _sum_rows(value):
    return jnp.sum(value, axis=0, keepdims=True)


def pallas_dist_mean_ax0_shard0_i_m1024_n512_kernel(x: jax.Array):
    m, n = x.shape
    wide_cols = n - _NARROW_COLS
    body_rows = m - _HEAD_ROWS - _STRIP_ROWS
    strip_start = m - _STRIP_ROWS
    wide_rows = _STRIP_ROWS - _WIDE_END_ROWS
    narrow_rows = _STRIP_ROWS - _NARROW_END_ROWS
    inv_count = 1.0 / (m * _N_DEV)

    def kernel_body(
        x_hbm,
        out_ref,
        body_buf,
        wide_buf,
        wide_end_buf,
        narrow_buf,
        narrow_end_buf,
        head_buf,
        wide_sum,
        narrow_sum,
        shard_sum,
        diag_head,
        diag_wide_sum,
        diag_narrow_sum,
        left_shard_sum,
        right_shard_sum,
        load_sems,
        send_sems,
        recv_sems,
    ):
        wide = pl.ds(0, wide_cols)
        narrow = pl.ds(wide_cols, _NARROW_COLS)
        head_hbm = x_hbm.at[pl.ds(0, _HEAD_ROWS)]

        loads = [
            pltpu.make_async_copy(src, dst, load_sems.at[j])
            for j, (src, dst) in enumerate((
                (x_hbm.at[pl.ds(_HEAD_ROWS, body_rows)], body_buf),
                (x_hbm.at[pl.ds(strip_start, wide_rows), wide], wide_buf),
                (x_hbm.at[pl.ds(m - _WIDE_END_ROWS, _WIDE_END_ROWS), wide], wide_end_buf),
                (x_hbm.at[pl.ds(strip_start, narrow_rows), narrow], narrow_buf),
                (x_hbm.at[pl.ds(m - _NARROW_END_ROWS, _NARROW_END_ROWS), narrow], narrow_end_buf),
                (head_hbm, head_buf),
            ))
        ]
        *early_loads, head_load = loads
        for load in early_loads:
            load.start()
        body_load, wide_load, wide_end_load, narrow_load, narrow_end_load = early_loads

        me = lax.axis_index(_AXIS)
        right, diagonal, left = ((me + k) & (_N_DEV - 1) for k in (1, 2, 3))

        barrier = pltpu.get_barrier_semaphore()
        for peer in (diagonal, right, left):
            pl.semaphore_signal(
                barrier, inc=1, device_id=(peer,), device_id_type=pl.DeviceIdType.MESH
            )
        pl.semaphore_wait(barrier, _N_DEV - 1)

        copies = [
            pltpu.make_async_remote_copy(
                src_ref=src,
                dst_ref=dst,
                send_sem=send_sems.at[j],
                recv_sem=recv_sems.at[j],
                device_id=(peer,),
                device_id_type=pl.DeviceIdType.MESH,
            )
            for j, (src, dst, peer) in enumerate((
                (head_hbm, diag_head, diagonal),
                (wide_sum, diag_wide_sum, diagonal),
                (narrow_sum, diag_narrow_sum, diagonal),
                (shard_sum, left_shard_sum, right),
                (shard_sum, right_shard_sum, left),
            ))
        ]
        head_copy, wide_copy, narrow_copy, rightward_copy, leftward_copy = copies
        head_copy.start()

        body_load.wait()
        acc = _fold_rows(body_buf)

        wide_load.wait()
        wide_acc = _fold_rows_onto(acc[:, :wide_cols], wide_buf)
        wide_end_load.wait()
        wide_total = _sum_rows(_fold_rows_onto(wide_acc, wide_end_buf))
        wide_sum[...] = wide_total
        wide_copy.start()

        narrow_load.wait()
        narrow_acc = _fold_rows_onto(acc[:, wide_cols:], narrow_buf)
        narrow_end_load.wait()
        narrow_total = _sum_rows(_fold_rows_onto(narrow_acc, narrow_end_buf))
        narrow_sum[...] = narrow_total
        narrow_copy.start()

        head_load.start()
        head_load.wait()
        total = jnp.concatenate([wide_total, narrow_total], axis=1)
        total = total + _sum_rows(_fold_rows(head_buf))
        shard_sum[...] = total
        rightward_copy.start()
        leftward_copy.start()

        for copy in copies:
            copy.wait_send()
        rightward_copy.wait_recv()
        leftward_copy.wait_recv()
        total = total + left_shard_sum[...] + right_shard_sum[...]
        head_copy.wait_recv()
        total = total + _sum_rows(_fold_rows(diag_head))
        wide_copy.wait_recv()
        out_ref[:, wide] = (total[:, :wide_cols] + diag_wide_sum[...]) * inv_count
        narrow_copy.wait_recv()
        out_ref[:, narrow] = (total[:, wide_cols:] + diag_narrow_sum[...]) * inv_count

    def vmem(*shape):
        return pltpu.VMEM(shape, jnp.float32)

    return pl.pallas_call(
        kernel_body,
        out_shape=jax.ShapeDtypeStruct((1, n), jnp.float32),
        in_specs=[pl.BlockSpec(memory_space=pl.ANY)],
        out_specs=pl.BlockSpec(memory_space=pltpu.VMEM),
        scratch_shapes=[
            vmem(body_rows, n),
            vmem(wide_rows, wide_cols),
            vmem(_WIDE_END_ROWS, wide_cols),
            vmem(narrow_rows, _NARROW_COLS),
            vmem(_NARROW_END_ROWS, _NARROW_COLS),
            vmem(_HEAD_ROWS, n),
            vmem(1, wide_cols),
            vmem(1, _NARROW_COLS),
            vmem(1, n),
            vmem(_HEAD_ROWS, n),
            vmem(1, wide_cols),
            vmem(1, _NARROW_COLS),
            vmem(1, n),
            vmem(1, n),
            pltpu.SemaphoreType.DMA((6,)),
            pltpu.SemaphoreType.DMA((5,)),
            pltpu.SemaphoreType.DMA((5,)),
        ],
        compiler_params=pltpu.CompilerParams(
            collective_id=0,
            disable_semaphore_checks=True,
        ),
    )(x)
```
